```python
import numpy as np

kernel_name = "dist_moe_shared_ep_outshard_n512_d256_e2_h512"

def setup_inputs():
    x = np.random.randn(512, 256).astype(np.float32)
    router_W = np.random.randn(256, 8).astype(np.float32) * 0.1
    scores64 = x.astype(np.float64) @ router_W.astype(np.float64)
    route_idx = np.argsort(-scores64, axis=-1)[:, :1].astype(np.int32)
    expert_W = np.random.randn(8, 256, 512).astype(np.float32) * 0.02
    shared_W = np.random.randn(256, 512).astype(np.float32) * 0.02
    return {"x": x, "router_W": router_W, "route_idx": route_idx, "expert_W": expert_W, "shared_W": shared_W}

def reference(x, router_W, route_idx, expert_W, shared_W):
    scores = x @ router_W
    s_max = scores.max(axis=-1, keepdims=True)
    probs = np.exp(scores - s_max)
    probs = probs / probs.sum(axis=-1, keepdims=True)
    shared = x @ shared_W
    out = np.zeros((512, 512), dtype=np.float32)
    for i in range(512):
        e = int(route_idx[i, 0])
        out[i] = shared[i] + probs[i, e] * (x[i] @ expert_W[e])
    return out
```

```python
import functools
import jax
import jax.numpy as jnp
from jax import lax
from jax.experimental import pallas as pl
from jax.experimental.pallas import tpu as pltpu

ND = 4
T = 128
D = 256
H = 512
CAP = 64
NR = 2
G = 16
HBM = pl.BlockSpec(memory_space=pltpu.HBM)
VM = pl.BlockSpec(memory_space=pltpu.VMEM)
f32 = jnp.float32
bf16 = jnp.bfloat16
i32 = jnp.int32


def make(NCH=4):
    CW = H // NCH

    def body(x_hbm, rwt_hbm, ri_hbm, ew_hbm, sw_hbm, out_ref,
             xb, rwb, rib, wb, swb, xcat, sbuf, rbuf, perm, pt,
             lsem, wsem, ssem, rsem):
        me = lax.axis_index("i")
        bar = pltpu.get_barrier_semaphore()
        for k in range(1, ND):
            pl.semaphore_signal(bar, 1, device_id=((me + k) & 3,), device_id_type=pl.DeviceIdType.MESH)

        c_ri = pltpu.make_async_copy(ri_hbm, rib, lsem.at[0]); c_ri.start()
        c_x = []
        for k in range(ND):
            off = pl.multiple_of(((me + k) & 3) * T, T)
            c = pltpu.make_async_copy(x_hbm.at[pl.ds(off, T)], xb.at[k], lsem.at[1 + k])
            c.start(); c_x.append(c)
        c_w = []
        for n in range(NCH):
            c = pltpu.make_async_copy(ew_hbm.at[:, :, pl.ds(n * CW, CW)], wb.at[n], wsem.at[n])
            c.start(); c_w.append(c)
        c_rw = pltpu.make_async_copy(rwt_hbm, rwb, lsem.at[5]); c_rw.start()
        c_sw = pltpu.make_async_copy(sw_hbm, swb, lsem.at[6]); c_sw.start()

        c_ri.wait()
        e = [rib[:, pl.ds(pl.multiple_of(((me + k) & 3) * T, T), T)] for k in range(ND)]
        row8 = lax.broadcasted_iota(i32, (8, T), 0)
        own = [(ek >> 1) == me for ek in e]
        ko = (me - (e[0] >> 1)) & 3
        A = jnp.zeros((8, T), f32)
        for k in range(ND):
            A = jnp.where((row8 == k) & own[k], 1.0, A)
        for j in range(1, ND):
            A = jnp.where((row8 == 3 + j) & (ko == j), 1.0, A)
        ti = lax.broadcasted_iota(i32, (T, 2 * T), 0)
        tj = lax.broadcasted_iota(i32, (T, 2 * T), 1)
        U = jnp.where((ti < tj) | (tj >= T), 1.0, 0.0).astype(bf16)
        PC = jnp.dot(A.astype(bf16), U, preferred_element_type=f32).astype(i32)
        P = PC[:, :T]
        cnt = [PC[r, T] for r in range(7)]
        cnt_send = cnt[0:4]
        cnt_recv = [cnt[0], cnt[4], cnt[5], cnt[6]]

        def nchunks(c, r):
            return (jnp.clip(c - CAP * r, 0, CAP) + (G - 1)) >> 4

        two_send = (cnt_send[0] > CAP) | (cnt_send[1] > CAP) | (cnt_send[2] > CAP) | (cnt_send[3] > CAP)
        two_recv = (cnt_recv[0] > CAP) | (cnt_recv[1] > CAP) | (cnt_recv[2] > CAP) | (cnt_recv[3] > CAP)

        row128 = lax.broadcasted_iota(i32, (T, T), 0)

        def compact(r):
            for k in range(ND):
                rk = P[k:k + 1, :] - CAP * r
                pos = jnp.where(own[k] & (rk >= 0) & (rk < CAP), rk + CAP * (e[k] & 1), -1)
                S = jnp.where(row128 == pos, 1.0, 0.0).astype(bf16)
                if r == 0:
                    c_x[k].wait()
                xs = jnp.dot(S, xb[k].astype(bf16), preferred_element_type=f32).astype(bf16)
                xcat[r, pl.ds(CAP * k, CAP), 0:D] = xs[0:CAP]
                xcat[r, pl.ds(CAP * k, CAP), D:2 * D] = xs[CAP:2 * CAP]

        def send_desc(r, n, k, c):
            rows = pl.ds(CAP * k, G * c)
            return pltpu.make_async_remote_copy(
                src_ref=sbuf.at[r, n, rows], dst_ref=rbuf.at[r, n, rows],
                send_sem=ssem.at[r, n, k - 1], recv_sem=rsem.at[r, n, k - 1],
                device_id=((me + k) & 3,), device_id_type=pl.DeviceIdType.MESH)

        def expert(r, n):
            w = wb[n].reshape(2 * D, CW).astype(bf16)
            y = jnp.dot(xcat[r], w, preferred_element_type=f32).astype(bf16)
            rbuf[r, n, 0:CAP] = y[0:CAP]
            sbuf[r, n, CAP:] = y[CAP:]

        def send(r, n):
            for k in (2, 1, 3):
                nc = nchunks(cnt_send[k], r)
                for c in range(1, CAP // G + 1):
                    @pl.when(nc == c)
                    def _():
                        send_desc(r, n, k, c).start()

        compact(0)
        for n in range(NCH):
            c_w[n].wait()
            expert(0, n)
            if n == 0:
                pl.semaphore_wait(bar, ND - 1)
            send(0, n)

        @pl.when(two_send)
        def _():
            compact(1)
            for n in range(NCH):
                expert(1, n)
                send(1, n)

        c_rw.wait()
        xo = xb[0].astype(bf16)
        sT = lax.dot_general(rwb[...].astype(bf16), xo, (((1,), (1,)), ((), ())), preferred_element_type=f32)
        m = jnp.max(sT, axis=0, keepdims=True)
        pe = jnp.exp(sT - m)
        pr = pe / jnp.sum(pe, axis=0, keepdims=True)
        p = jnp.sum(jnp.where(row8 == e[0], pr, 0.0), axis=0, keepdims=True)
        pt[...] = jnp.broadcast_to(p, (T, T)).T
        rank = P[0:1, :]
        for j in range(1, ND):
            rank = jnp.where(ko == j, P[3 + j:4 + j, :], rank)

        def build_perm(r):
            rk = rank - CAP * r
            kidx = jnp.where((rk >= 0) & (rk < CAP), ko * CAP + rk, -1)
            KT = jnp.broadcast_to(kidx, (T, T)).T
            lane = lax.broadcasted_iota(i32, (T, T), 1)
            perm[r, :, 0:T] = jnp.where(KT == lane, 1.0, 0.0).astype(bf16)
            perm[r, :, T:2 * T] = jnp.where(KT == lane + T, 1.0, 0.0).astype(bf16)

        build_perm(0)
        c_sw.wait()
        out_ref[...] = jnp.dot(xo, swb[...].astype(bf16), preferred_element_type=f32)

        rowi = lax.broadcasted_iota(i32, (ND * CAP, CW), 0)

        def combine(r, n):
            for k in (1, 3, 2):
                nc = nchunks(cnt_recv[k], r)
                for c in range(1, CAP // G + 1):
                    @pl.when(nc == c)
                    def _():
                        send_desc(r, n, k, c).wait_recv()
            lim = jnp.where(rowi < CAP, cnt_recv[0], jnp.where(rowi < 2 * CAP, cnt_recv[1], jnp.where(rowi < 3 * CAP, cnt_recv[2], cnt_recv[3])))
            valid = ((rowi & (CAP - 1)) + CAP * r) < lim
            rb = jnp.where(valid, rbuf[r, n].astype(f32), 0.0).astype(bf16)
            acc = jnp.dot(perm[r], rb, preferred_element_type=f32)
            for h in range(CW // T):
                cols = pl.ds(n * CW + h * T, T)
                out_ref[:, cols] = out_ref[:, cols] + pt[...] * acc[:, h * T:(h + 1) * T]

        for n in range(NCH):
            combine(0, n)

        @pl.when(two_recv)
        def _():
            build_perm(1)
            for n in range(NCH):
                combine(1, n)

        def drain(r):
            for n in range(NCH):
                for k in (2, 1, 3):
                    nc = nchunks(cnt_send[k], r)
                    for c in range(1, CAP // G + 1):
                        @pl.when(nc == c)
                        def _():
                            send_desc(r, n, k, c).wait_send()
        drain(0)

        @pl.when(two_send)
        def _():
            drain(1)

    def kernel(x, router_W, route_idx, expert_W, shared_W):
        return pl.pallas_call(
            body,
            out_shape=jax.ShapeDtypeStruct((T, H), f32),
            in_specs=[HBM] * 5,
            out_specs=VM,
            scratch_shapes=[
                pltpu.VMEM((ND, T, D), f32),
                pltpu.VMEM((8, D), f32),
                pltpu.VMEM((1, ND * T), i32),
                pltpu.VMEM((NCH, 2, D, CW), f32),
                pltpu.VMEM((D, H), f32),
                pltpu.VMEM((NR, ND * CAP, 2 * D), bf16),
                pltpu.VMEM((NR, NCH, ND * CAP, CW), bf16),
                pltpu.VMEM((NR, NCH, ND * CAP, CW), bf16),
                pltpu.VMEM((NR, T, ND * CAP), bf16),
                pltpu.VMEM((T, T), f32),
                pltpu.SemaphoreType.DMA((7,)),
                pltpu.SemaphoreType.DMA((NCH,)),
                pltpu.SemaphoreType.DMA((NR, NCH, ND - 1)),
                pltpu.SemaphoreType.DMA((NR, NCH, ND - 1)),
            ],
            compiler_params=pltpu.CompilerParams(collective_id=0),
        )(x, router_W.T, route_idx.reshape(1, ND * T), expert_W, shared_W)
    return kernel

pallas_dist_moe_shared_ep_outshard_n512_d256_e2_h512_kernel = make(2)
```

```python
import jax
import jax.numpy as jnp
from jax import lax
from jax.experimental import pallas as pl
from jax.experimental.pallas import tpu as pltpu

ND = 4
T = 128
D = 256
H = 512
NT = H // 128
CAP = 64
NR = 2
G = 8
LG = 3

CHUNKS = ((0, 2), (2, 1), (3, 1), (2, 2))
NCH = 3
POS = {2: 0, 1: 1, 3: 2}
SLOT = {1: 0, 3: 1, 2: 2}

f32, bf16, i32 = jnp.float32, jnp.bfloat16, jnp.int32
MESH = pl.DeviceIdType.MESH


def _dot(a, b):
    return jnp.dot(a, b, preferred_element_type=f32)


def _when_eq(v, nmax, fn):
    for a in range(nmax // 8, -1, -1):
        @pl.when((v >> 3) == a)
        def _():
            for c in range(min(8 * a + 7, nmax), max(8 * a, 1) - 1, -1):
                pl.when(v == c)(lambda c=c: fn(c))


def _pieces(g, gmax, fn):
    b = gmax
    while b >= 1:
        pl.when((g & b) != 0)(lambda b=b: fn(b, g & ~(2 * b - 1)))
        b //= 2


def _kernel(x_hbm, rwt_hbm, ri_hbm, ew_hbm, sw_hbm, out_ref,
            xb, rwb, rib, wb, swb, xcat, sbuf, rbuf, zbuf, perm, lsem, rsem):
    me = lax.axis_index("i")
    peer = lambda k: ((me + k) & 3,)
    ssem = lsem.at[0]

    def x_copy(k, s):
        off = pl.multiple_of(((me + k) & 3) * T, T)
        return pltpu.make_async_copy(x_hbm.at[pl.ds(off, T)], xb.at[k], lsem.at[s])

    def w_copy(n):
        cols = pl.ds(CHUNKS[n][0] * 128, CHUNKS[n][1] * 128)
        return pltpu.make_async_copy(ew_hbm.at[:, :, cols], wb.at[:, :, cols], lsem.at[3 + n])

    ld_a = [pltpu.make_async_copy(ri_hbm, rib, lsem.at[0]), x_copy(2, 0)]
    ld_b = [x_copy(1, 1), x_copy(3, 1)]
    ld_c = [x_copy(0, 2), pltpu.make_async_copy(rwt_hbm, rwb, lsem.at[2]),
            pltpu.make_async_copy(sw_hbm, swb, lsem.at[2])]
    ld_w = [w_copy(n) for n in range(NCH)]
    for c in (*ld_a, ld_w[0], *ld_b, ld_w[1], ld_w[2], *ld_c):
        c.start()

    bar = pltpu.get_barrier_semaphore()
    for k in range(1, ND):
        pl.semaphore_signal(bar, 1, device_id=peer(k), device_id_type=MESH)
    zbuf[...] = jnp.zeros_like(zbuf)

    for c in ld_a:
        c.wait()
    e = [rib[:, pl.ds(pl.multiple_of(((me + k) & 3) * T, T), T)] & 7 for k in range(ND)]
    row8 = lax.broadcasted_iota(i32, (8, T), 0)
    own = [(ek >> 1) == me for ek in e]
    ko = (me - (e[0] >> 1)) & 3
    A = jnp.zeros((8, T), f32)
    for k in range(1, ND):
        A = jnp.where((row8 == k - 1) & own[k], 1.0, A)
        A = jnp.where((row8 == 2 + k) & (ko == k), 1.0, A)
    ti = lax.broadcasted_iota(i32, (T, 2 * T), 0)
    tj = lax.broadcasted_iota(i32, (T, 2 * T), 1)
    U = jnp.where((ti < tj) | (tj >= T), 1.0, 0.0).astype(bf16)
    PC = _dot(A.astype(bf16), U).astype(i32)
    P = PC[:, :T]
    cs = {k: PC[k - 1, T] for k in range(1, ND)}
    cr = {k: PC[2 + k, T] for k in range(1, ND)}

    def ngran(c, r):
        return (jnp.clip(c - CAP * r, 0, CAP) + (G - 1)) >> LG

    def recv_groups(r, k):
        if r == 1:
            return [(0, NT, rsem.at[NCH + 1])]
        if k == 2:
            return [(*CHUNKS[n], rsem.at[n]) for n in range(NCH)]
        return [(0, NT, rsem.at[NCH])]

    def zero_fill(r):
        ng = CAP // G
        for k in (2, 1, 3):
            def piece(b, hi, k=k):
                row = pl.multiple_of(CAP * SLOT[k] + (ng - b - hi) * G, G)
                for t0, nt, sem in recv_groups(r, k):
                    pltpu.make_async_copy(
                        zbuf.at[pl.ds(0, nt), pl.ds(0, b * G)],
                        rbuf.at[r, pl.ds(t0, nt), pl.ds(row, b * G)], sem).start()
            _pieces(ng - ngran(cr[k], r), ng, piece)

    def compact(r, k):
        row = lax.broadcasted_iota(i32, (T, T), 0)
        rk = P[k - 1:k, :] - CAP * r
        pos = jnp.where(own[k] & (rk >= 0) & (rk < CAP), rk + CAP * (e[k] & 1), -1)
        S = jnp.where(row == pos, 1.0, 0.0).astype(bf16)
        rows = pl.ds(CAP * POS[k], CAP)
        for h in range(D // 128):
            xs = _dot(S, xb[k, :, h * 128:(h + 1) * 128].astype(bf16)).astype(bf16)
            xcat[h, rows, :] = xs[:CAP]
            xcat[2 + h, rows, :] = xs[CAP:]

    def expert(r, n, ks):
        t0, nt = CHUNKS[n]
        lo, m = CAP * min(POS[k] for k in ks), CAP * len(ks)
        cols = pl.ds(t0 * 128, nt * 128)
        y = None
        for kt in range(4):
            w = wb[kt // 2, pl.ds((kt % 2) * 128, 128), cols].astype(bf16)
            t = _dot(xcat[kt, pl.ds(lo, m), :], w)
            y = t if y is None else y + t
        y = y.astype(bf16)
        for j in range(nt):
            sbuf[t0 + j, pl.ds(3 * CAP * r + lo, m), :] = y[:, j * 128:(j + 1) * 128]

    def send(r, n, k):
        t0, nt = CHUNKS[n]
        if isinstance(k, str):
            first = (me & 1) == (0 if k == "y" else 1)
            kk = jnp.where(first, 1, 3)
            src = jnp.where(first, CAP * POS[1], CAP * POS[3])
            dst = jnp.where(first, CAP * SLOT[1], CAP * SLOT[3])
            cnt = jnp.where(first, cs[1], cs[3])
        else:
            kk, src, dst, cnt = k, CAP * POS[k], CAP * SLOT[k], cs[k]
        sem = rsem.at[NCH + 1] if r == 1 else rsem.at[n] if k == 2 else rsem.at[NCH]

        def piece(b, hi):
            s0 = pl.multiple_of(3 * CAP * r + src + hi * G, G)
            d0 = pl.multiple_of(dst + hi * G, G)
            pltpu.make_async_remote_copy(
                src_ref=sbuf.at[pl.ds(t0, nt), pl.ds(s0, b * G)],
                dst_ref=rbuf.at[r, pl.ds(t0, nt), pl.ds(d0, b * G)],
                send_sem=ssem, recv_sem=sem, device_id=peer(kk), device_id_type=MESH).start()
        _pieces(ngran(cnt, r), CAP // G, piece)

    def drain(r):
        g = sum(ngran(cs[k], r) for k in range(1, ND))

        def wait(c):
            v = sbuf.at[:, pl.ds(0, G * c)]
            pltpu.make_async_remote_copy(
                src_ref=v, dst_ref=v, send_sem=ssem, recv_sem=rsem.at[0],
                device_id=(me,), device_id_type=MESH).wait_send()
        _when_eq(g, 3 * CAP // G, wait)

    def wait_recv(v, sem):
        pltpu.make_async_copy(v, v, sem).wait()

    compact(0, 2)
    zero_fill(0)
    ld_w[0].wait()
    expert(0, 0, (2,))
    pl.semaphore_wait(bar, ND - 1)
    send(0, 0, 2)
    for c in ld_b:
        c.wait()
    compact(0, 1)
    compact(0, 3)
    expert(0, 0, (1, 3))
    send(0, 0, "y")
    ld_w[1].wait()
    expert(0, 1, (2,))
    send(0, 1, 2)
    ld_w[2].wait()
    expert(0, 2, (2,))
    send(0, 2, 2)
    send(0, 0, "x")
    expert(0, 3, (1, 3))
    send(0, 3, "y")
    send(0, 3, "x")

    for c in ld_c:
        c.wait()
    xo = xb[0]
    xob = xo.astype(bf16)
    sT = lax.dot_general(rwb[...], xo, (((1,), (1,)), ((), ())),
                         precision=lax.Precision.HIGHEST, preferred_element_type=f32)
    pe = jnp.exp(sT - jnp.max(sT, axis=0, keepdims=True))
    pr = pe / jnp.sum(pe, axis=0, keepdims=True)
    p = jnp.sum(jnp.where(row8 == e[0], pr, 0.0), axis=0, keepdims=True)
    PT = jnp.broadcast_to(p, (T, T)).T
    rank = jnp.where(ko == 1, P[3:4, :], jnp.where(ko == 2, P[4:5, :], P[5:6, :]))
    slot = jnp.where(ko == 1, SLOT[1], jnp.where(ko == 2, SLOT[2], SLOT[3]))
    lane = lax.broadcasted_iota(i32, (T, T), 1)

    def build_perm(r):
        rk = rank - CAP * r
        code = jnp.where(ko == 0, 4 * CAP + (e[0] & 1),
                         jnp.where((rk >= 0) & (rk < CAP), slot * CAP + rk, -1))
        CT = jnp.broadcast_to(code, (T, T)).T
        for s in range(2):
            perm[s] = jnp.where(CT == lane + s * T, PT, 0.0).astype(bf16)
        return CT

    CT = build_perm(0)
    acc = _dot(xob, swb[...].astype(bf16))
    for j in range(2):
        g = jnp.where(CT == 4 * CAP + j, PT, 0.0)
        for h in range(D // 128):
            lhs = (xo[:, h * 128:(h + 1) * 128] * g).astype(bf16)
            acc = acc + _dot(lhs, wb[j, h * 128:(h + 1) * 128, :].astype(bf16))
    out_ref[...] = acc

    def combine_nbr(r):
        for j in range(NT):
            out_ref[:, j * 128:(j + 1) * 128] += _dot(perm[0], rbuf[r, j, 0:T, :])

    def combine_diag(r, t0, nt):
        ms = 4 // nt
        mr = T // ms
        for j in range(t0, t0 + nt):
            rb = rbuf[r, j, T:T + CAP, :]
            for i in range(ms):
                out_ref[i * mr:(i + 1) * mr, j * 128:(j + 1) * 128] += _dot(
                    perm[1, i * mr:(i + 1) * mr, 0:CAP], rb)

    def recv_diag(n):
        t0, nt = CHUNKS[n]
        wait_recv(rbuf.at[0, pl.ds(t0, nt), pl.ds(T, CAP)], rsem.at[n])
        combine_diag(0, t0, nt)

    recv_diag(0)
    wait_recv(rbuf.at[0, :, pl.ds(0, T)], rsem.at[NCH])
    combine_nbr(0)
    recv_diag(1)
    drain(0)
    recv_diag(2)

    @pl.when((cs[1] > CAP) | (cs[2] > CAP) | (cs[3] > CAP))
    def _():
        for k in (2, 1, 3):
            compact(1, k)
        for n in range(NCH):
            expert(1, n, (2, 1, 3))
            for k in (2, 1, 3):
                send(1, n, k)
        drain(1)

    @pl.when((cr[1] > CAP) | (cr[2] > CAP) | (cr[3] > CAP))
    def _():
        zero_fill(1)
        build_perm(1)
        wait_recv(rbuf.at[1], rsem.at[NCH + 1])
        combine_nbr(1)
        combine_diag(1, 0, NT)


def pallas_dist_moe_shared_ep_outshard_n512_d256_e2_h512_kernel(
    x: jax.Array,
    router_W: jax.Array,
    route_idx: jax.Array,
    expert_W: jax.Array,
    shared_W: jax.Array,
):
    hbm = pl.BlockSpec(memory_space=pltpu.HBM)
    return pl.pallas_call(
        _kernel,
        out_shape=jax.ShapeDtypeStruct((T, H), f32),
        in_specs=[hbm] * 5,
        out_specs=pl.BlockSpec(memory_space=pltpu.VMEM),
        scratch_shapes=[
            pltpu.VMEM((ND, T, D), f32),
            pltpu.VMEM((8, D), f32),
            pltpu.VMEM((1, ND * T), i32),
            pltpu.VMEM((2, D, H), f32),
            pltpu.VMEM((D, H), f32),
            pltpu.VMEM((4, 3 * CAP, 128), bf16),
            pltpu.VMEM((NT, NR * 3 * CAP, 128), bf16),
            pltpu.VMEM((NR, NT, 3 * CAP, 128), bf16),
            pltpu.VMEM((NT, CAP, 128), bf16),
            pltpu.VMEM((2, T, T), bf16),
            pltpu.SemaphoreType.DMA((3 + NCH,)),
            pltpu.SemaphoreType.DMA((NCH + 2,)),
        ],
        compiler_params=pltpu.CompilerParams(collective_id=0),
    )(x, router_W.T, route_idx.reshape(1, ND * T), expert_W, shared_W)
```

```python
import jax
import jax.numpy as jnp
from jax import lax
from jax.experimental import pallas as pl
from jax.experimental.pallas import tpu as pltpu

ND = 4
T = 128
D = 256
H = 512
NT = H // 128
CAP = 64
NR = 2
G = 4
LG = 2

CHUNKS = ((0, 2), (2, 1), (3, 1), (2, 2))
NCH = 3
POS = {2: 0, 1: 1, 3: 2}
SLOT = {1: 0, 3: 1, 2: 2}

f32, bf16, i32 = jnp.float32, jnp.bfloat16, jnp.int32
MESH = pl.DeviceIdType.MESH


def _dot(a, b):
    return jnp.dot(a, b, preferred_element_type=f32)


def _when_eq(v, nmax, fn):
    for a in range(nmax // 8, -1, -1):
        @pl.when((v >> 3) == a)
        def _():
            for c in range(min(8 * a + 7, nmax), max(8 * a, 1) - 1, -1):
                pl.when(v == c)(lambda c=c: fn(c))


def _pieces(g, gmax, fn):
    b = gmax
    while b >= 1:
        pl.when((g & b) != 0)(lambda b=b: fn(b, g & ~(2 * b - 1)))
        b //= 2


def _kernel(x_hbm, rwt_hbm, ri_hbm, ew_hbm, sw_hbm, out_ref,
            xb, rwb, rib, wb, swb, xcat, sbuf, rbuf, zbuf, perm, lsem, rsem):
    me = lax.axis_index("i")
    peer = lambda k: ((me + k) & 3,)
    ssem = lsem.at[0]

    def x_copy(k, s):
        off = pl.multiple_of(((me + k) & 3) * T, T)
        return pltpu.make_async_copy(x_hbm.at[pl.ds(off, T)], xb.at[k], lsem.at[s])

    def w_copy(n):
        cols = pl.ds(CHUNKS[n][0] * 128, CHUNKS[n][1] * 128)
        return pltpu.make_async_copy(ew_hbm.at[:, :, cols], wb.at[:, :, cols], lsem.at[3 + n])

    ld_a = [pltpu.make_async_copy(ri_hbm, rib, lsem.at[0]), x_copy(2, 0)]
    ld_b = [x_copy(1, 1), x_copy(3, 1)]
    ld_c = [x_copy(0, 2), pltpu.make_async_copy(rwt_hbm, rwb, lsem.at[2]),
            pltpu.make_async_copy(sw_hbm, swb, lsem.at[2])]
    ld_w = [w_copy(n) for n in range(NCH)]
    for c in (*ld_a, ld_w[0], *ld_b, ld_w[1], ld_w[2], *ld_c):
        c.start()

    bar = pltpu.get_barrier_semaphore()
    for k in range(1, ND):
        pl.semaphore_signal(bar, 1, device_id=peer(k), device_id_type=MESH)
    zbuf[...] = jnp.zeros_like(zbuf)

    for c in ld_a:
        c.wait()
    e = [rib[:, pl.ds(pl.multiple_of(((me + k) & 3) * T, T), T)] & 7 for k in range(ND)]
    row8 = lax.broadcasted_iota(i32, (8, T), 0)
    own = [(ek >> 1) == me for ek in e]
    ko = (me - (e[0] >> 1)) & 3
    A = jnp.zeros((8, T), f32)
    for k in range(1, ND):
        A = jnp.where((row8 == k - 1) & own[k], 1.0, A)
        A = jnp.where((row8 == 2 + k) & (ko == k), 1.0, A)
    ti = lax.broadcasted_iota(i32, (T, 2 * T), 0)
    tj = lax.broadcasted_iota(i32, (T, 2 * T), 1)
    U = jnp.where((ti < tj) | (tj >= T), 1.0, 0.0).astype(bf16)
    PC = _dot(A.astype(bf16), U).astype(i32)
    P = PC[:, :T]
    cs = {k: PC[k - 1, T] for k in range(1, ND)}
    cr = {k: PC[2 + k, T] for k in range(1, ND)}

    def ngran(c, r):
        return (jnp.clip(c - CAP * r, 0, CAP) + (G - 1)) >> LG

    def recv_groups(r, k):
        if r == 1:
            return [(0, NT, rsem.at[NCH + 1])]
        if k == 2:
            return [(*CHUNKS[n], rsem.at[n]) for n in range(NCH)]
        return [(0, NT, rsem.at[NCH])]

    def zero_fill(r):
        ng = CAP // G
        for k in (2, 1, 3):
            def piece(b, hi, k=k):
                row = pl.multiple_of(CAP * SLOT[k] + (ng - b - hi) * G, G)
                for t0, nt, sem in recv_groups(r, k):
                    pltpu.make_async_copy(
                        zbuf.at[pl.ds(0, nt), pl.ds(0, b * G)],
                        rbuf.at[r, pl.ds(t0, nt), pl.ds(row, b * G)], sem).start()
            _pieces(ng - ngran(cr[k], r), ng, piece)

    def compact(r, k):
        row = lax.broadcasted_iota(i32, (T, T), 0)
        rk = P[k - 1:k, :] - CAP * r
        pos = jnp.where(own[k] & (rk >= 0) & (rk < CAP), rk + CAP * (e[k] & 1), -1)
        S = jnp.where(row == pos, 1.0, 0.0).astype(bf16)
        rows = pl.ds(CAP * POS[k], CAP)
        for h in range(D // 128):
            xs = _dot(S, xb[k, :, h * 128:(h + 1) * 128].astype(bf16)).astype(bf16)
            xcat[h, rows, :] = xs[:CAP]
            xcat[2 + h, rows, :] = xs[CAP:]

    def expert(r, n, ks):
        t0, nt = CHUNKS[n]
        lo, m = CAP * min(POS[k] for k in ks), CAP * len(ks)
        cols = pl.ds(t0 * 128, nt * 128)
        y = None
        for kt in range(4):
            w = wb[kt // 2, pl.ds((kt % 2) * 128, 128), cols].astype(bf16)
            t = _dot(xcat[kt, pl.ds(lo, m), :], w)
            y = t if y is None else y + t
        y = y.astype(bf16)
        for j in range(nt):
            sbuf[t0 + j, pl.ds(3 * CAP * r + lo, m), :] = y[:, j * 128:(j + 1) * 128]

    def send(r, n, k):
        t0, nt = CHUNKS[n]
        if isinstance(k, str):
            first = (me & 1) == (0 if k == "y" else 1)
            kk = jnp.where(first, 1, 3)
            src = jnp.where(first, CAP * POS[1], CAP * POS[3])
            dst = jnp.where(first, CAP * SLOT[1], CAP * SLOT[3])
            cnt = jnp.where(first, cs[1], cs[3])
        else:
            kk, src, dst, cnt = k, CAP * POS[k], CAP * SLOT[k], cs[k]
        sem = rsem.at[NCH + 1] if r == 1 else rsem.at[n] if k == 2 else rsem.at[NCH]

        def piece(b, hi):
            s0 = pl.multiple_of(3 * CAP * r + src + hi * G, G)
            d0 = pl.multiple_of(dst + hi * G, G)
            pltpu.make_async_remote_copy(
                src_ref=sbuf.at[pl.ds(t0, nt), pl.ds(s0, b * G)],
                dst_ref=rbuf.at[r, pl.ds(t0, nt), pl.ds(d0, b * G)],
                send_sem=ssem, recv_sem=sem, device_id=peer(kk), device_id_type=MESH).start()
        _pieces(ngran(cnt, r), CAP // G, piece)

    def drain(r):
        g = sum(ngran(cs[k], r) for k in range(1, ND))

        def wait(c):
            v = sbuf.at[:, pl.ds(0, G * c)]
            pltpu.make_async_remote_copy(
                src_ref=v, dst_ref=v, send_sem=ssem, recv_sem=rsem.at[0],
                device_id=(me,), device_id_type=MESH).wait_send()
        _when_eq(g, 3 * CAP // G, wait)

    def wait_recv(v, sem):
        pltpu.make_async_copy(v, v, sem).wait()

    compact(0, 2)
    zero_fill(0)
    ld_w[0].wait()
    expert(0, 0, (2,))
    pl.semaphore_wait(bar, ND - 1)
    send(0, 0, 2)
    for c in ld_b:
        c.wait()
    compact(0, 1)
    compact(0, 3)
    expert(0, 0, (1, 3))
    send(0, 0, "y")
    ld_w[1].wait()
    expert(0, 1, (2,))
    send(0, 1, 2)
    ld_w[2].wait()
    expert(0, 2, (2,))
    send(0, 2, 2)
    send(0, 0, "x")
    expert(0, 3, (1, 3))
    send(0, 3, "y")
    send(0, 3, "x")

    for c in ld_c:
        c.wait()
    xo = xb[0]
    xob = xo.astype(bf16)
    rw = rwb[...]
    rwh, xol = rw.astype(bf16), (xo - xob.astype(f32)).astype(bf16)
    rwl = (rw - rwh.astype(f32)).astype(bf16)
    nt_dot = lambda a, b: lax.dot_general(a, b, (((1,), (1,)), ((), ())), preferred_element_type=f32)
    sT = nt_dot(rwh, xob) + nt_dot(rwl, xob) + nt_dot(rwh, xol)
    pe = jnp.exp(sT - jnp.max(sT, axis=0, keepdims=True))
    pr = pe / jnp.sum(pe, axis=0, keepdims=True)
    p = jnp.sum(jnp.where(row8 == e[0], pr, 0.0), axis=0, keepdims=True)
    PT = jnp.broadcast_to(p, (T, T)).T
    rank = jnp.where(ko == 1, P[3:4, :], jnp.where(ko == 2, P[4:5, :], P[5:6, :]))
    slot = jnp.where(ko == 1, SLOT[1], jnp.where(ko == 2, SLOT[2], SLOT[3]))
    lane = lax.broadcasted_iota(i32, (T, T), 1)

    def build_perm(r):
        rk = rank - CAP * r
        code = jnp.where(ko == 0, 4 * CAP + (e[0] & 1),
                         jnp.where((rk >= 0) & (rk < CAP), slot * CAP + rk, -1))
        CT = jnp.broadcast_to(code, (T, T)).T
        for s in range(2):
            perm[s] = jnp.where(CT == lane + s * T, PT, 0.0).astype(bf16)
        return CT

    CT = build_perm(0)
    yl = None
    for j in range(2):
        for h in range(D // 128):
            lhs = jnp.where(CT == 4 * CAP + j, xo[:, h * 128:(h + 1) * 128], 0.0).astype(bf16)
            t = _dot(lhs, wb[j, h * 128:(h + 1) * 128, :].astype(bf16))
            yl = t if yl is None else yl + t
    sh = _dot(xob, swb[...].astype(bf16))
    for j in range(NT):
        out_ref[:, j * 128:(j + 1) * 128] = sh[:, j * 128:(j + 1) * 128] + PT * yl[:, j * 128:(j + 1) * 128]

    def combine_nbr(r):
        for j in range(NT):
            out_ref[:, j * 128:(j + 1) * 128] += _dot(perm[0], rbuf[r, j, 0:T, :])

    def combine_diag(r, t0, nt):
        ms = 4 // nt
        mr = T // ms
        for j in range(t0, t0 + nt):
            rb = rbuf[r, j, T:T + CAP, :]
            for i in range(ms):
                out_ref[i * mr:(i + 1) * mr, j * 128:(j + 1) * 128] += _dot(
                    perm[1, i * mr:(i + 1) * mr, 0:CAP], rb)

    def recv_diag(n):
        t0, nt = CHUNKS[n]
        wait_recv(rbuf.at[0, pl.ds(t0, nt), pl.ds(T, CAP)], rsem.at[n])
        combine_diag(0, t0, nt)

    drain(0)
    recv_diag(0)
    wait_recv(rbuf.at[0, :, pl.ds(0, T)], rsem.at[NCH])
    wait_recv(rbuf.at[0, pl.ds(2, 1), pl.ds(T, CAP)], rsem.at[1])
    combine_nbr(0)
    combine_diag(0, 2, 1)
    recv_diag(2)

    @pl.when((cs[1] > CAP) | (cs[2] > CAP) | (cs[3] > CAP))
    def _():
        for k in (2, 1, 3):
            compact(1, k)
        for n in range(NCH):
            expert(1, n, (2, 1, 3))
            for k in (2, 1, 3):
                send(1, n, k)
        drain(1)

    @pl.when((cr[1] > CAP) | (cr[2] > CAP) | (cr[3] > CAP))
    def _():
        zero_fill(1)
        build_perm(1)
        wait_recv(rbuf.at[1], rsem.at[NCH + 1])
        combine_nbr(1)
        combine_diag(1, 0, NT)


def pallas_dist_moe_shared_ep_outshard_n512_d256_e2_h512_kernel(
    x: jax.Array,
    router_W: jax.Array,
    route_idx: jax.Array,
    expert_W: jax.Array,
    shared_W: jax.Array,
):
    hbm = pl.BlockSpec(memory_space=pltpu.HBM)
    return pl.pallas_call(
        _kernel,
        out_shape=jax.ShapeDtypeStruct((T, H), f32),
        in_specs=[hbm] * 5,
        out_specs=pl.BlockSpec(memory_space=pltpu.VMEM),
        scratch_shapes=[
            pltpu.VMEM((ND, T, D), f32),
            pltpu.VMEM((8, D), f32),
            pltpu.VMEM((1, ND * T), i32),
            pltpu.VMEM((2, D, H), f32),
            pltpu.VMEM((D, H), f32),
            pltpu.VMEM((4, 3 * CAP, 128), bf16),
            pltpu.VMEM((NT, NR * 3 * CAP, 128), bf16),
            pltpu.VMEM((NR, NT, 3 * CAP, 128), bf16),
            pltpu.VMEM((NT, CAP, 128), bf16),
            pltpu.VMEM((2, T, T), bf16),
            pltpu.SemaphoreType.DMA((3 + NCH,)),
            pltpu.SemaphoreType.DMA((NCH + 2,)),
        ],
        compiler_params=pltpu.CompilerParams(collective_id=0),
    )(x, router_W.T, route_idx.reshape(1, ND * T), expert_W, shared_W)
```
